```python
import numpy as np

kernel_name = "dist_moe_cap_ep_n512_d256_e4_h512"

def setup_inputs():
    x = np.random.randn(512, 256).astype(np.float32)
    router_W = np.random.randn(256, 16).astype(np.float32) * 0.1
    scores64 = x.astype(np.float64) @ router_W.astype(np.float64)
    route_idx = np.argsort(-scores64, axis=-1)[:, :1].astype(np.int32)
    expert_W = np.random.randn(16, 256, 512).astype(np.float32) * 0.02
    return {"x": x, "router_W": router_W, "route_idx": route_idx, "expert_W": expert_W}

def reference(x, router_W, route_idx, expert_W):
    counts = np.zeros(16, dtype=np.int64)
    out = np.zeros((512, 512), dtype=np.float32)
    for i in range(512):
        e = int(route_idx[i, 0])
        if counts[e] < 25:
            out[i] = x[i] @ expert_W[e]
            counts[e] += 1
    return out
```

```python
import contextlib

import jax
import jax.numpy as jnp
from jax import lax
from jax.experimental import pallas as pl
from jax.experimental.pallas import tpu as pltpu

N_DEV = 4
N_TOK = 512
D_IN = 256
D_OUT = 512
N_EXP = 16
E_LOC = N_EXP // N_DEV
CAP = 25
ROWS = 32
LANE = 128
N_HALF = 2 * E_LOC - 1
N_PIECE = N_HALF + 2
MESH = pl.DeviceIdType.MESH


def make(scopes=False, n_fwd=3, unroll_rows=CAP):
    scope = jax.named_scope if scopes else (lambda name: contextlib.nullcontext())

    def body(x_hbm, r_hbm, w_hbm, out_ref, r_v, w_v, xs_v, tok_v, tok_s, dst_v, dst_s,
             yh_v, yq_v, misc_sem, w_sem, x_sem, send_sem, recv_sem):
        me = lax.axis_index("i")
        right = (me + 1) & 3
        left = (me + 3) & 3

        def w_copy(p):
            if p < N_HALF:
                e, cols = p // 2, pl.ds((p % 2) * 2 * LANE, 2 * LANE)
            else:
                e, cols = E_LOC - 1, pl.ds((p - N_HALF + 2) * LANE, LANE)
            return pltpu.make_async_copy(
                w_hbm.at[e, :, cols], w_v.at[e, :, cols], w_sem.at[p])

        def piece(k, p):
            if isinstance(p, int) and p >= N_HALF:
                return yq_v.at[k, p - N_HALF, pl.ds(0, CAP + 1)]
            return yh_v.at[k, p, pl.ds(0, CAP)]

        def send(k, p, dst):
            kd = (me + k - dst) & 3
            return pltpu.make_async_remote_copy(
                piece(k, p), piece(kd, p), send_sem, recv_sem.at[kd * N_PIECE + p],
                device_id=(dst,), device_id_type=MESH)

        def wait_recv(k, p):
            pltpu.make_async_remote_copy(
                piece(k, p), piece(k, p), send_sem, recv_sem.at[k * N_PIECE + p],
                device_id=(me,), device_id_type=MESH).wait_recv()

        def wait_send(p):
            pltpu.make_async_remote_copy(
                piece(0, p), piece(0, p), send_sem, recv_sem.at[0],
                device_id=(me,), device_id_type=MESH).wait_send()

        with scope("start"):
            route_copy = pltpu.make_async_copy(r_hbm, r_v, misc_sem.at[0])
            route_copy.start()
            for p in range(N_PIECE):
                w_copy(p).start(priority=1)
            barrier = pltpu.get_barrier_semaphore()
            for dst in (right, left):
                pl.semaphore_signal(barrier, 1, device_id=(dst,), device_id_type=MESH)

            @pl.when(me == 0)
            def _():
                pl.semaphore_signal(barrier, 1, device_id=(2,), device_id_type=MESH)

        with scope("zero"):
            out_ref[...] = jnp.zeros(out_ref.shape, out_ref.dtype)
            for e in range(E_LOC):
                xs_v[e, pl.ds(ROWS - 8, 8), :] = jnp.zeros((8, D_IN), jnp.float32)

        with scope("wait_route"):
            route_copy.wait()

        with scope("cum"):
            route = (r_v[...] - E_LOC * me) & (N_EXP - 1)
            expert = lax.broadcasted_iota(jnp.int32, (N_EXP, LANE), 0)
            lhs = []
            before = jnp.zeros((N_EXP, LANE), jnp.float32)
            for b in range(N_TOK // LANE):
                hit = jnp.where(route[b:b + 1, :] == expert, 1.0, 0.0)
                lhs.append(jnp.concatenate([hit, before], axis=1))
                before = before + hit
            lhs.append(jnp.concatenate([jnp.zeros_like(before), before], axis=1))
            lhs = jnp.concatenate(lhs, axis=0).astype(jnp.bfloat16)
            i = lax.broadcasted_iota(jnp.int32, (2 * LANE, LANE), 0)
            j = lax.broadcasted_iota(jnp.int32, (2 * LANE, LANE), 1)
            upto = jnp.where((i <= j) | (i >= LANE), 1.0, 0.0).astype(jnp.bfloat16)
            cum = jnp.dot(lhs, upto, preferred_element_type=jnp.float32)
            slot = lax.broadcasted_iota(jnp.int32, (ROWS, LANE), 0).astype(jnp.float32)

            def tokens_before(k):
                per_expert = []
                for e in range(k * E_LOC, (k + 1) * E_LOC):
                    n = jnp.zeros((ROWS, LANE), jnp.float32)
                    for b in range(N_TOK // LANE):
                        row = b * N_EXP + e
                        n = n + jnp.where(cum[row:row + 1, :] <= slot, 1.0, 0.0)
                    per_expert.append(n)
                return jnp.concatenate(per_expert, axis=0).astype(jnp.bfloat16)

            nt = (((1,), (1,)), ((), ()))
            tok = lax.dot_general(jnp.ones((8, LANE), jnp.bfloat16), tokens_before(0), nt,
                                  preferred_element_type=jnp.float32)
            tok_v[...] = jnp.minimum(tok, N_TOK - 1.0).astype(jnp.int32)
            tok_copy = pltpu.make_async_copy(tok_v.at[pl.ds(0, 1)], tok_s, misc_sem.at[1])
            tok_copy.start()

        with scope("dst"):
            row = lax.broadcasted_iota(jnp.int32, (8, LANE), 0)
            lane = lax.broadcasted_iota(jnp.int32, (8, LANE), 1)
            dst = jnp.where(row == 0, tok, float(N_TOK))
            for k in range(1, N_DEV):
                t = lax.dot_general(jnp.ones((8, LANE), jnp.bfloat16), tokens_before(k), nt,
                                    preferred_element_type=jnp.float32)
                dst = jnp.where(row == k, t, dst)
            over = jnp.where((lane & (ROWS - 1)) >= CAP, dst, float(N_TOK))
            dropped = jnp.min(jnp.min(over, axis=1, keepdims=True), axis=0, keepdims=True)
            dst = jnp.where(dst < N_TOK, dst, dropped).astype(jnp.int32)
            dst_v[...] = ((dst >> 3) << 5) | (dst & 7)
            dst_copy = pltpu.make_async_copy(dst_v.at[pl.ds(0, N_DEV)], dst_s, misc_sem.at[2])
            dst_copy.start()

        with scope("wait_tok"):
            tok_copy.wait()

        def row_copy(e, r, t):
            return pltpu.make_async_copy(
                x_hbm.at[pl.ds(t, 1)], xs_v.at[e, pl.ds(r, 1)], x_sem.at[e])

        for e in range(E_LOC):
            with scope(f"gather{e}"):
                for r in range(CAP):
                    row_copy(e, r, tok_s[0, e * ROWS + r]).start()

        for p in range(N_PIECE):
            e = min(p // 2, E_LOC - 1)
            if p % 2 == 0 and p < 2 * E_LOC:
                with scope(f"wait_x{e}"):
                    for r in range(CAP):
                        row_copy(e, r, 0).wait()
                    xs = xs_v[e].astype(jnp.bfloat16)
                    row = N_TOK // LANE * N_EXP + e
                    used = slot < jnp.minimum(cum[row:row + 1, :], float(CAP))
            with scope(f"wait_w{p}"):
                w_copy(p).wait()
            with scope(f"mm{p}"):
                if p < N_HALF:
                    w = w_v[e, :, pl.ds((p % 2) * 2 * LANE, 2 * LANE)]
                    y = jnp.dot(xs, w.astype(jnp.bfloat16), preferred_element_type=jnp.float32)
                    bits = []
                    for c in range(2):
                        v = jnp.where(used, y[:, c * LANE:(c + 1) * LANE], 0.0)
                        v = v.astype(jnp.bfloat16).astype(jnp.float32)
                        bits.append(lax.bitcast_convert_type(v, jnp.uint32))
                    yh_v[0, p] = (bits[0] >> 16) | bits[1]
                else:
                    w = w_v[e, :, pl.ds((p - N_HALF + 2) * LANE, LANE)]
                    y = jnp.dot(xs, w.astype(jnp.bfloat16), preferred_element_type=jnp.float32)
                    yq_v[0, p - N_HALF] = jnp.where(used, y, 0.0).astype(jnp.bfloat16)
            if p == 0:
                with scope("barrier"):
                    pl.semaphore_wait(barrier, jnp.where(me == 2, 3, 2))
            with scope(f"send{p}"):
                first = left if p < n_fwd else jnp.where(me == 2, 0, left)
                send(0, p, first).start()
                send(0, p, right).start()

        with scope("extra"):
            @pl.when(me == 2)
            def _():
                for p in range(n_fwd, N_PIECE):
                    send(0, p, 1).start()

            @pl.when(me == 3)
            def _():
                for p in range(n_fwd):
                    wait_recv(3, p)
                    send(3, p, 0).start()

        with scope("wait_dst"):
            dst_copy.wait()

        def scatter_half(k, p):
            e = p // 2
            col = (p % 2) * 16
            words = yh_v[k, p]
            lo = lax.bitcast_convert_type(words << 16, jnp.float32)
            hi = lax.bitcast_convert_type(words & jnp.uint32(0xFFFF0000), jnp.float32)
            for r in range(CAP):
                t = dst_s[k, e * ROWS + r] + col
                out_ref[pl.ds(t, 1), :] = lo[r:r + 1, :]
                out_ref[pl.ds(t + 8, 1), :] = hi[r:r + 1, :]

        def scatter_quarter(k, q):
            v = yq_v[k, q].astype(jnp.float32)
            for r in range(CAP):
                t = dst_s[k, (E_LOC - 1) * ROWS + r]
                out_ref[pl.ds(t + (2 + q) * 8, 1), :] = v[r:r + 1, :]

        k1 = jnp.where(me == 1, 3, 1)
        k2 = jnp.where((me == 0) | (me == 2), 3, 2)
        k3 = jnp.where(me == 1, 1, jnp.where(me == 3, 3, 2))

        def forward(k, p, first_source):
            is_low = p < E_LOC
            to = jnp.where(me == 0, jnp.where(first_source, 3, 1), 2)
            go = (me == 0) | (first_source & (((me == 1) & is_low) | ((me == 3) & ~is_low)))

            @pl.when(go)
            def _():
                send(k, p, to).start()

        def half_step(s, _):
            own = s < N_HALF
            last = s >= 3 * N_HALF
            mid = s - N_HALF
            p = jnp.where(own, s, jnp.where(last, s - 3 * N_HALF, mid >> 1))
            first_source = (mid & 1) == 0
            k = jnp.where(own, 0, jnp.where(last, k3, jnp.where(first_source, k1, k2)))

            @pl.when(~own & ~(last & (me == 3) & (p < n_fwd)))
            def _():
                wait_recv(k, p)

            @pl.when(~own & ~last)
            def _():
                forward(k, p, first_source)

            scatter_half(k, p)

        def quarter_step(s, _):
            k = jnp.where(s == 0, 0, jnp.where(s == 1, k1, k2))
            for q in range(2):
                @pl.when(s > 0)
                def _():
                    wait_recv(k, N_HALF + q)
                    forward(k, N_HALF + q, s == 1)

                scatter_quarter(k, q)

        with scope("own"):
            lax.fori_loop(0, N_HALF, half_step, None)
        with scope("mid"):
            lax.fori_loop(N_HALF, 3 * N_HALF, half_step, None)
        with scope("quart"):
            lax.fori_loop(0, 3, quarter_step, None)
        with scope("last"):
            lax.fori_loop(3 * N_HALF, 4 * N_HALF, half_step, None)
        with scope("wq0"):
            wait_recv(k3, N_HALF)
        with scope("sq0"):
            scatter_quarter(k3, 0)

        with scope("wait_send"):
            n_half = jnp.where(me == 0, 4 * N_HALF, jnp.where(
                me == 1, 2 * N_HALF + E_LOC, jnp.where(
                    me == 2, 3 * N_HALF - n_fwd, 3 * N_HALF - E_LOC + n_fwd)))
            n_quarter = jnp.where(me == 0, 8, jnp.where(me == 1, 4, 6))
            lax.fori_loop(0, n_half, lambda *_: wait_send(0), None)
            lax.fori_loop(0, n_quarter, lambda *_: wait_send(N_HALF), None)

        with scope("wq1"):
            wait_recv(k3, N_HALF + 1)
        with scope("sq1"):
            scatter_quarter(k3, 1)

    def fn(x, router_W, route_idx, expert_W):
        del router_W
        hbm = pl.BlockSpec(memory_space=pltpu.HBM)
        out = pl.pallas_call(
            body,
            out_shape=jax.ShapeDtypeStruct((N_TOK * D_OUT // LANE, LANE), jnp.float32),
            in_specs=[hbm, hbm, hbm],
            out_specs=pl.BlockSpec(memory_space=pltpu.VMEM),
            scratch_shapes=[
                pltpu.VMEM((N_TOK // LANE, LANE), jnp.int32),
                pltpu.VMEM((E_LOC, D_IN, D_OUT), jnp.float32),
                pltpu.VMEM((E_LOC, ROWS, D_IN), jnp.float32),
                pltpu.VMEM((8, LANE), jnp.int32),
                pltpu.SMEM((1, LANE), jnp.int32),
                pltpu.VMEM((8, LANE), jnp.int32),
                pltpu.SMEM((N_DEV, LANE), jnp.int32),
                pltpu.VMEM((N_DEV, N_HALF, ROWS, LANE), jnp.uint32),
                pltpu.VMEM((N_DEV, 2, ROWS, LANE), jnp.bfloat16),
                pltpu.SemaphoreType.DMA((3,)),
                pltpu.SemaphoreType.DMA((N_PIECE,)),
                pltpu.SemaphoreType.DMA((E_LOC,)),
                pltpu.SemaphoreType.DMA,
                pltpu.SemaphoreType.DMA((N_DEV * N_PIECE,)),
            ],
            compiler_params=pltpu.CompilerParams(
                collective_id=0,
                disable_bounds_checks=True,
                disable_semaphore_checks=True,
            ),
        )(x, route_idx.reshape(N_TOK // LANE, LANE), expert_W)
        out = out.reshape(N_TOK // 8, D_OUT // LANE, 8, LANE).transpose(0, 2, 1, 3)
        return out.reshape(N_TOK, D_OUT)

    return fn


pallas_dist_moe_cap_ep_n512_d256_e4_h512_kernel = make()
```

```python
import contextlib

import jax
import jax.numpy as jnp
from jax import lax
from jax.experimental import pallas as pl
from jax.experimental.pallas import tpu as pltpu

N_DEV = 4
N_TOK = 512
D_IN = 256
D_OUT = 512
N_EXP = 16
E_LOC = N_EXP // N_DEV
CAP = 25
ROWS = 32
LANE = 128
N_BLK = N_TOK // LANE
MESH = pl.DeviceIdType.MESH
A, B, C, D = range(N_DEV)

Q4 = ((0, 0, 2), (0, 2, 2), (1, 0, 2), (1, 2, 2), (2, 0, 2), (2, 2, 2),
      (3, 0, 1), (3, 2, 1), (3, 1, 1), (3, 3, 1))
Q6 = ((0, 0, 2), (0, 2, 2), (1, 0, 2), (1, 2, 2), (2, 0, 2), (2, 2, 1), (2, 3, 1),
      (3, 0, 1), (3, 2, 1), (3, 1, 1), (3, 3, 1))
Q6b = ((0, 0, 2), (0, 2, 2), (1, 0, 2), (1, 2, 2), (2, 0, 2), (2, 3, 1), (2, 2, 1),
       (3, 0, 1), (3, 2, 1), (3, 1, 1), (3, 3, 1))
Q6c = ((0, 0, 2), (0, 2, 2), (1, 0, 2), (1, 2, 2), (2, 0, 2), (2, 2, 1), (3, 0, 1),
       (2, 3, 1), (3, 1, 1), (3, 3, 1), (3, 2, 1))
LAYOUTS = dict(Q4=Q4, Q6=Q6, Q6b=Q6b, Q6c=Q6c)


def make(scopes=False, probe=None, layout="Q6", fwd=(0, 2, 3, 4), last_order=(1, 0, 5, 2, 6, 7, 3, 8, 9, 4, 10, 4),
         n_send_wait=4, g2_early=True, cut_q=0, cut_h=16, split=0, defer=True):
    scope = jax.named_scope if scopes else (lambda name: contextlib.nullcontext())
    pieces = LAYOUTS[layout]
    n_piece = len(pieces)
    every = list(range(n_piece))
    halves = [p for p in every if pieces[p][2] == 2]
    quarters = [p for p in every if pieces[p][2] == 1]
    low = [p for p in every if pieces[p][0] < E_LOC // 2]
    whole = (0, CAP)
    opens, closes = quarters[0::2], quarters[1::2]
    parts = []
    for p in every:
        if p == every[-1] and cut_q:
            parts += [(p, (0, cut_q), False), (p, (cut_q, CAP), False)]
        elif p == fwd[-1] and cut_h:
            parts += [(p, (0, cut_h), True), (p, (cut_h, CAP), True)]
        elif p == fwd[0] and split:
            parts += [(p, (0, split), False), (p, (split, CAP), True)]
        else:
            parts.append((p, whole, p in fwd))
    if last_order is None:
        last_order = {10: (0, 1, 5, 2, 6, 3, 7, 8, 4, 9)}.get(
            n_piece, (0, 1, 5, 2, 6, 7, 3, 8, 9, 4, 10))
    order = []
    for p in last_order:
        todo = [i for i, part in enumerate(parts) if part[0] == p and i not in order]
        order += todo[:1] if last_order.count(p) > 1 else todo

    def body(x_hbm, r_hbm, w_hbm, out_ref, r_v, wf_v, wh_v, wq_v, xs_v, dst_v, dst_s,
             yh_v, yq_v, dst_sem, in_sem, x_sem, send_sem, recv_sem, part_sem, fence_sem):
        def w_copy(p):
            e, c, n = pieces[p]
            if e == 0:
                return pltpu.make_async_copy(w_hbm.at[0], wf_v, in_sem.at[0])
            dst = wh_v.at[halves.index(p) - 2] if n == 2 else wq_v.at[quarters.index(p)]
            return pltpu.make_async_copy(
                w_hbm.at[e, :, pl.ds(c * LANE, n * LANE)], dst, in_sem.at[p])

        with scope("start"):
            route_copy = pltpu.make_async_copy(r_hbm, r_v, in_sem.at[1])
            route_copy.start()
            for p in range(1, n_piece):
                w_copy(p).start(priority=1)

            me = lax.axis_index("i")
            right = (me + 1) & 3
            left = (me + 3) & 3
            barrier = pltpu.get_barrier_semaphore()
            for dst in (right, left):
                pl.semaphore_signal(barrier, 1, device_id=(dst,), device_id_type=MESH)

            @pl.when(me == A)
            def _():
                pl.semaphore_signal(barrier, 1, device_id=(C,), device_id_type=MESH)

        def fence():
            pl.semaphore_signal(fence_sem, 1)
            pl.semaphore_wait(fence_sem, 1)

        def piece(k, p, slots=whole):
            lo, hi = slots
            if p in quarters:
                hi += (hi % 2) * (1 if p in closes else -1)
                return yq_v.at[k, quarters.index(p), pl.ds(lo, hi - lo)]
            return yh_v.at[k, halves.index(p), pl.ds(lo, hi - lo)]

        def remote(k, p, dst, kd, slots=whole, sem=None):
            sem = recv_sem.at[kd * n_piece + p] if sem is None else sem
            return pltpu.make_async_remote_copy(
                piece(k, p, slots), piece(kd, p, slots), send_sem, sem,
                device_id=(dst,), device_id_type=MESH)

        def wait_recv(k, p):
            remote(k, p, me, k).wait_recv()

        def part_copy(k, i):
            p, slots, _ = parts[i]
            return remote(k, p, A, 3, slots, None if slots == whole else part_sem.at[i])

        with scope("zero"):
            out_ref[...] = jnp.zeros(out_ref.shape, out_ref.dtype)
            for e in range(E_LOC):
                for c in range(2):
                    xs_v[e, c, pl.ds(ROWS - 8, 8), :] = jnp.zeros((8, LANE), jnp.float32)
            i = lax.broadcasted_iota(jnp.int32, (2 * LANE, LANE), 0)
            j = lax.broadcasted_iota(jnp.int32, (2 * LANE, LANE), 1)
            upto = jnp.where((i <= j) | (i >= LANE), 1.0, 0.0).astype(jnp.bfloat16)
            slot = lax.broadcasted_iota(jnp.int32, (ROWS, LANE), 0).astype(jnp.float32)

        def running_counts(first, second):
            row = lax.broadcasted_iota(jnp.int32, (8, LANE), 0)
            expert = jnp.where(row < E_LOC, first, second) * E_LOC + (row & (E_LOC - 1))
            lhs = []
            before = jnp.zeros((8, LANE), jnp.float32)
            for b in range(N_BLK):
                hit = jnp.where(route[b:b + 1, :] == expert, 1.0, 0.0)
                lhs.append(jnp.concatenate([hit, before], axis=1))
                before = before + hit
            lhs = jnp.concatenate(lhs, axis=0).astype(jnp.bfloat16)
            return jnp.dot(lhs, upto, preferred_element_type=jnp.float32)

        def tokens_before(cum, e):
            n = None
            for b in range(N_BLK):
                t = jnp.where(cum[8 * b + e:8 * b + e + 1, :] <= slot, 1.0, 0.0)
                n = t if n is None else n + t
            return n

        with scope("wait_route"):
            route_copy.wait()

        route = r_v[...] & (N_EXP - 1)
        cum_near = running_counts(me, jnp.where((me & 1) == 0, B, A))

        def row_copy(e, r, t):
            return pltpu.make_async_copy(
                x_hbm.at[t >> 3, :, pl.ds(t & 7, 1)], xs_v.at[e, :, pl.ds(r, 1)], x_sem.at[e])

        used = {}
        src = {}

        def locate(e):
            tok = jnp.sum(tokens_before(cum_near, e), axis=1, keepdims=True)
            used[e] = jnp.broadcast_to(tok, (ROWS, LANE)) < N_TOK
            src[e] = jnp.minimum(tok, N_TOK - 1.0).astype(jnp.int32)

        def gather(e):
            if e not in src:
                locate(e)
            for r in range(CAP):
                row_copy(e, r, src[e][r, 0]).start()

        xs = {}

        def wait_gather(e):
            with scope(f"wait_x{e}"):
                for r in range(CAP):
                    row_copy(e, r, 0).wait()
            xs[e] = jnp.concatenate([xs_v[e, 0], xs_v[e, 1]], axis=1).astype(jnp.bfloat16)

        def wait_w(p):
            with scope(f"wait_w{p}"):
                w_copy(p).wait()

        dst_copies = [
            pltpu.make_async_copy(dst_v.at[k], dst_s.at[pl.ds(k * LANE, LANE)], dst_sem)
            for k in range(N_DEV)]

        def table():
            cum_far = running_counts(jnp.where(me == D, B, D), jnp.where(me == C, A, C))
            nt = (((1,), (1,)), ((), ()))
            row = lax.broadcasted_iota(jnp.int32, (8, LANE), 0)
            lane = lax.broadcasted_iota(jnp.int32, (8, LANE), 1)
            dst = jnp.full((8, LANE), float(N_TOK), jnp.float32)
            for k in range(N_DEV):
                cum = cum_near if k < 2 else cum_far
                n = [tokens_before(cum, (k % 2) * E_LOC + e) for e in range(E_LOC)]
                n = jnp.concatenate(n, axis=0).astype(jnp.bfloat16)
                t = lax.dot_general(jnp.ones((8, LANE), jnp.bfloat16), n, nt,
                                    preferred_element_type=jnp.float32)
                dst = jnp.where(row == k, t, dst)
            over = jnp.where((lane & (ROWS - 1)) >= CAP, dst, float(N_TOK))
            dropped = jnp.min(jnp.min(over, axis=0, keepdims=True), axis=1, keepdims=True)
            dst = jnp.where(dst < N_TOK, dst, dropped).astype(jnp.int32)
            dst_v[...] = ((dst >> 3) << 5) | (dst & 7)
            for c in dst_copies:
                c.start()

        my_slot = jnp.where(me == C, 3, jnp.where(me == D, 2, 1))
        direct = [p for p, slots, relayed in parts if not relayed and slots == whole]

        odd = [None]

        def compute(p):
            e, c, n = pieces[p]
            if n == 2:
                w = wf_v[:, pl.ds(c * LANE, 2 * LANE)] if e == 0 else wh_v[halves.index(p) - 2]
                y = jnp.dot(xs[e], w.astype(jnp.bfloat16), preferred_element_type=jnp.float32)
                bits = []
                for b in range(2):
                    v = jnp.where(used[e], y[:, b * LANE:(b + 1) * LANE], 0.0)
                    v = v.astype(jnp.bfloat16).astype(jnp.float32)
                    bits.append(lax.bitcast_convert_type(v, jnp.uint32))
                yh_v[0, halves.index(p)] = (bits[0] >> 16) | bits[1]
            else:
                w = wq_v[quarters.index(p)].astype(jnp.bfloat16)
                y = jnp.dot(xs[e], w, preferred_element_type=jnp.float32)
                y = jnp.where(used[e], y, 0.0)
                if p in opens:
                    odd[0] = jnp.broadcast_to(y[CAP - 1:CAP], (8, LANE))
                else:
                    y = jnp.concatenate(
                        [y[:ROWS - 8], jnp.where(slot[ROWS - 8:] == CAP, odd[0], y[ROWS - 8:])])
                yq_v[0, quarters.index(p)] = y.astype(jnp.bfloat16)
            if p == 0:
                pl.when(me == A)(table)
                pl.semaphore_wait(barrier, jnp.where(me == C, 3, 2))
            for i, (q, slots, relayed) in enumerate(parts):
                if q == p and not relayed and slots != whole:
                    pl.when(me == C)(lambda: part_copy(0, i).start())
            if p in direct:
                remote(0, p, jnp.where(me == C, A, left), my_slot).start()
            elif p in fwd and not (split and p == fwd[0]):
                remote(0, p, left, my_slot).start()
            else:
                pl.when(me != C)(lambda: remote(0, p, left, my_slot).start())
            if defer and p not in fwd and p < fwd[-1]:
                pl.when(me != C)(lambda: remote(0, p, right, my_slot).start())
            else:
                remote(0, p, right, my_slot).start()
            if defer and p == fwd[-1]:
                for q in range(p):
                    if q not in fwd:
                        pl.when(me == C)(lambda: remote(0, q, D, 3).start())

        gather(0)
        fence()
        gather(1)
        if g2_early:
            gather(2)
        else:
            locate(2)
        locate(3)
        wait_w(0)
        wait_gather(0)
        compute(0)
        fence()
        compute(1)
        if not g2_early:
            fence()
            gather(2)
        wait_gather(1)
        wait_w(2)
        compute(2)
        if g2_early:
            wait_gather(2)
        else:
            fence()
        gather(3)
        for p in range(3, n_piece):
            if pieces[p][0] not in xs:
                wait_gather(pieces[p][0])
            wait_w(p)
            compute(p)

        with scope("extra"):
            @pl.when(me == D)
            def _():
                for p in fwd:
                    wait_recv(3, p)
                    for i, (q, slots, relayed) in enumerate(parts):
                        if q == p and relayed:
                            part_copy(3, i).start()
                    if p == fwd[-3] and probe is None:
                        for q in every:
                            if q not in low:
                                wait_recv(1, q)
                                remote(1, q, C, 3).start()

            @pl.when(me == B)
            def _():
                for p in low:
                    wait_recv(1, p)
                    remote(1, p, C, 3).start()

            @pl.when(me == C)
            def _():
                for p in every:
                    if p not in fwd or (split and p == fwd[0]):
                        remote(0, p, B, 3).start()

        pl.when(me != A)(table)

        with scope("wait_dst"):
            for c in dst_copies:
                c.wait()

        def wait_sends(sent):
            for d in range(N_DEV):
                @pl.when(me == d)
                def _():
                    for p, slots in sorted(sent[d], key=lambda s: (s[0] in opens, s[1])):
                        remote(0, p, me, 0, slots).wait_send()

        own = [(p, whole) for p in every]
        from_c = [(p, s) for p, s, relayed in parts if not relayed]
        from_d = [(p, s) for p, s, relayed in parts if relayed]
        if probe is not None:
            @pl.when(me == A)
            def _():
                for k, p in probe:
                    with jax.named_scope(f"probe{k}_{p}"):
                        wait_recv(k, p)
                for k in (1, 2, 3):
                    for p in every:
                        if (k, p) not in probe:
                            wait_recv(k, p)

            for d, ks in ((B, (1, 3)), (C, (1, 2)), (D, (1, 3))):
                @pl.when(me == d)
                def _():
                    for k in ks:
                        for p in every:
                            if not (d == D and k == 3 and p in fwd) and not (
                                    d == B and k == 1 and p in low):
                                wait_recv(k, p)
                    if d == C:
                        for p in low:
                            wait_recv(3, p)
            wait_sends((2 * own, 2 * own + [own[p] for p in low], 2 * own + from_c,
                        2 * own + from_d))
            return

        def scatter(k, p, slots=whole):
            e, c, n = pieces[p]
            first = k * LANE + e * ROWS
            lo, hi = slots
            if n == 1:
                v = yq_v[k, quarters.index(p)].astype(jnp.float32)
                for r in range(lo, min(hi, CAP - 1) if p in opens else hi):
                    out_ref[pl.ds(dst_s[first + r] + 8 * c, 1), :] = v[r:r + 1, :]
                if p in closes and hi == CAP:
                    e, c, _ = pieces[opens[closes.index(p)]]
                    t = dst_s[k * LANE + e * ROWS + CAP - 1]
                    out_ref[pl.ds(t + 8 * c, 1), :] = v[CAP:CAP + 1, :]
                return
            words = yh_v[k, halves.index(p), pl.ds(lo, hi - lo)]
            v = pltpu.bitcast(words, jnp.bfloat16).astype(jnp.float32)
            for r in range(hi - lo):
                out_ref[pl.ds(dst_s[first + lo + r] + 8 * c, 2, stride=8), :] = v[2 * r:2 * r + 2, :]

        with scope("mid"):
            for p in every:
                wait_recv(2, p)
                pl.when(me == A)(lambda: remote(2, p, B, 2).start())
                pl.when(me != (B if p in low else D))(lambda: wait_recv(1, p))
                pl.when(me == A)(lambda: remote(1, p, D, 2).start())
                for k in range(3):
                    scatter(k, p)

        done = set()
        for n, i in enumerate(order):
            p, slots, relayed = parts[i]
            if n == len(order) - n_send_wait:
                with scope("wait_send"):
                    wait_sends((4 * own, 2 * own + [own[p] for p in low], 2 * own + from_c,
                                2 * own + [own[p] for p in every if p not in low] + from_d))
            with scope(f"lw{p}_{i}"):
                if slots != whole:
                    pl.when(me == A)(lambda: part_copy(3, i).wait_recv())
                    if p not in done:
                        others = (me != A) & (me != D) if p in fwd else me != A
                        pl.when(others)(lambda: wait_recv(3, p))
                elif p in fwd:
                    pl.when(me != D)(lambda: wait_recv(3, p))
                else:
                    wait_recv(3, p)
                done.add(p)
            with scope(f"ls{p}_{i}"):
                scatter(3, p, slots)

    def fn(x, router_W, route_idx, expert_W):
        del router_W
        hbm = pl.BlockSpec(memory_space=pltpu.HBM)
        x = x.reshape(N_TOK // 8, 8, D_IN // LANE, LANE).transpose(0, 2, 1, 3)
        out = pl.pallas_call(
            body,
            out_shape=jax.ShapeDtypeStruct((N_TOK * D_OUT // LANE, LANE), jnp.float32),
            in_specs=[hbm, hbm, hbm],
            out_specs=pl.BlockSpec(memory_space=pltpu.VMEM),
            scratch_shapes=[
                pltpu.VMEM((N_BLK, LANE), jnp.int32),
                pltpu.VMEM((D_IN, D_OUT), jnp.float32),
                pltpu.VMEM((len(halves) - 2, D_IN, 2 * LANE), jnp.float32),
                pltpu.VMEM((len(quarters), D_IN, LANE), jnp.float32),
                pltpu.VMEM((E_LOC, 2, ROWS, LANE), jnp.float32),
                pltpu.VMEM((8, LANE), jnp.int32),
                pltpu.SMEM((N_DEV * LANE,), jnp.int32),
                pltpu.VMEM((N_DEV, len(halves), ROWS, LANE), jnp.uint32),
                pltpu.VMEM((N_DEV, len(quarters), ROWS, LANE), jnp.bfloat16),
                pltpu.SemaphoreType.DMA,
                pltpu.SemaphoreType.DMA((n_piece,)),
                pltpu.SemaphoreType.DMA((E_LOC,)),
                pltpu.SemaphoreType.DMA,
                pltpu.SemaphoreType.DMA((N_DEV * n_piece,)),
                pltpu.SemaphoreType.DMA((len(parts),)),
                pltpu.SemaphoreType.REGULAR,
            ],
            compiler_params=pltpu.CompilerParams(
                collective_id=0,
                disable_bounds_checks=True,
                disable_semaphore_checks=True,
            ),
        )(x, route_idx.reshape(N_BLK, LANE), expert_W)
        out = out.reshape(N_TOK // 8, D_OUT // LANE, 8, LANE).transpose(0, 2, 1, 3)
        return out.reshape(N_TOK, D_OUT)

    return fn


pallas_dist_moe_cap_ep_n512_d256_e4_h512_kernel = make()
```

```python
import jax
import jax.numpy as jnp
from jax import lax
from jax.experimental import pallas as pl
from jax.experimental.pallas import tpu as pltpu

N_DEV = 4
N_TOK = 512
D_IN = 256
D_OUT = 512
N_EXP = 16
CAP = 25
E_LOC = N_EXP // N_DEV
SUB, LANE = 8, 128
ROWS = 32
N_BLK = N_TOK // LANE
A, B, C, D = range(N_DEV)

WIDE = ((0, 0), (0, 2), (1, 0), (1, 2), (2, 0))
NARROW = ((2, 3), (2, 2), (3, 0), (3, 2), (3, 1), (3, 3))
PIECES = WIDE + NARROW
N_PIECE = len(PIECES)

A_TO_C_VIA_B = (0, 1, 2, 3)
C_TO_A_VIA_D = (0, 2, 3, 4)
LAST_SLOT_ORDER = (1, 0, 5, 2, 6, 7, 3, 8, 9, 4, 10)


def _moe_kernel(x_hbm, route_hbm, w_hbm, out_ref,
                route_v, w_first, w_wide, w_narrow, xs_v, dst_v, dst_s, y_wide, y_narrow,
                in_sem, x_sem, dst_sem, send_sem, recv_sem, fence_sem):
    def w_copy(p):
        e, c = PIECES[p]
        if e == 0:
            return pltpu.make_async_copy(w_hbm.at[0], w_first, in_sem.at[1])
        if p < len(WIDE):
            return pltpu.make_async_copy(
                w_hbm.at[e, :, pl.ds(c * LANE, 2 * LANE)], w_wide.at[p - 2], in_sem.at[p])
        return pltpu.make_async_copy(
            w_hbm.at[e, :, pl.ds(c * LANE, LANE)], w_narrow.at[p - len(WIDE)], in_sem.at[p])

    def load_other_weights():
        for p in range(2, N_PIECE):
            w_copy(p).start(priority=1)

    route_copy = pltpu.make_async_copy(route_hbm, route_v, in_sem.at[0])
    route_copy.start()
    w_copy(0).start(priority=1)
    me = lax.axis_index("i")
    pl.when(me != B)(load_other_weights)

    right, left = (me + 1) & 3, (me + 3) & 3
    barrier = pltpu.get_barrier_semaphore()

    def greet(chip):
        pl.semaphore_signal(barrier, 1, device_id=(chip,), device_id_type=pl.DeviceIdType.MESH)

    greet(right)
    greet(left)
    pl.when(me == A)(lambda: greet(C))

    def fence():
        pl.semaphore_signal(fence_sem, 1)
        pl.semaphore_wait(fence_sem, 1)

    out_ref[...] = jnp.zeros(out_ref.shape, out_ref.dtype)
    for e in range(E_LOC):
        for c in range(D_IN // LANE):
            xs_v[e, c, pl.ds(ROWS - SUB, SUB), :] = jnp.zeros((SUB, LANE), jnp.float32)

    i = lax.broadcasted_iota(jnp.int32, (2 * LANE, LANE), 0)
    j = lax.broadcasted_iota(jnp.int32, (2 * LANE, LANE), 1)
    upto = jnp.where((i <= j) | (i >= LANE), 1.0, 0.0)
    rank = lax.broadcasted_iota(jnp.int32, (ROWS, LANE), 0).astype(jnp.float32)

    route_copy.wait()
    route = route_v[...] & (N_EXP - 1)

    def counts_of_expert(expert):
        hit = jnp.where(route == expert, 1.0, 0.0)
        blk = lax.broadcasted_iota(jnp.int32, hit.shape, 0)
        earlier = sum(jnp.where(blk > b, hit[b:b + 1], 0.0) for b in range(N_BLK - 1))
        counts = jnp.dot(jnp.concatenate([hit, earlier], axis=1), upto,
                         preferred_element_type=jnp.float32)
        return [counts[b:b + 1] for b in range(N_BLK)]

    def counts_of_chips(first, second):
        row = lax.broadcasted_iota(jnp.int32, (SUB, LANE), 0)
        expert = jnp.where(row < E_LOC, first, second) * E_LOC + (row & (E_LOC - 1))
        lhs = []
        earlier = jnp.zeros((SUB, LANE), jnp.float32)
        for b in range(N_BLK):
            hit = jnp.where(route[b:b + 1] == expert, 1.0, 0.0)
            lhs.append(jnp.concatenate([hit, earlier], axis=1))
            earlier = earlier + hit
        counts = jnp.dot(jnp.concatenate(lhs).astype(jnp.bfloat16), upto.astype(jnp.bfloat16),
                         preferred_element_type=jnp.float32)
        return [[counts[SUB * b + e:SUB * b + e + 1] for b in range(N_BLK)] for e in range(SUB)]

    def tokens_before(counts):
        return sum(jnp.where(n <= rank, 1.0, 0.0) for n in counts)

    token = {}

    def locate(e, counts):
        token[e] = jnp.sum(tokens_before(counts), axis=1, keepdims=True)

    def row_copy(e, r, t):
        return pltpu.make_async_copy(
            x_hbm.at[t >> 3, :, pl.ds(t & 7, 1)], xs_v.at[e, :, pl.ds(r, 1)], x_sem.at[e])

    def fetch_rows(e):
        t = jnp.minimum(token[e], N_TOK - 1.0).astype(jnp.int32)
        for r in range(CAP):
            row_copy(e, r, t[r, 0]).start()

    xs = {}

    def wait_rows(e):
        for r in range(CAP):
            row_copy(e, r, 0).wait()
        xs[e] = jnp.concatenate([xs_v[e, 0], xs_v[e, 1]], axis=1).astype(jnp.bfloat16)

    dst_copies = [
        pltpu.make_async_copy(dst_v.at[k], dst_s.at[pl.ds(k * LANE, LANE)], dst_sem)
        for k in range(N_DEV)]

    def find_output_rows():
        counts = near + counts_of_chips(jnp.where(me == D, B, D), jnp.where(me == C, A, C))
        row = lax.broadcasted_iota(jnp.int32, (SUB, LANE), 0)
        lane = lax.broadcasted_iota(jnp.int32, (SUB, LANE), 1)
        dst = jnp.full((SUB, LANE), float(N_TOK), jnp.float32)
        for k in range(N_DEV):
            n = [tokens_before(counts[k * E_LOC + e]) for e in range(E_LOC)]
            t = lax.dot_general(
                jnp.ones((SUB, LANE), jnp.bfloat16), jnp.concatenate(n).astype(jnp.bfloat16),
                (((1,), (1,)), ((), ())), preferred_element_type=jnp.float32)
            dst = jnp.where(row == k, t, dst)
        full = jnp.where((lane & (ROWS - 1)) >= CAP, dst, float(N_TOK))
        dropped = jnp.min(jnp.min(full, axis=0, keepdims=True), axis=1, keepdims=True)
        dst = jnp.where(dst < N_TOK, dst, dropped).astype(jnp.int32)
        dst_v[...] = (dst >> 3) * (SUB * D_OUT // LANE) + (dst & 7)
        for copy in dst_copies:
            copy.start()

    def carries_odd_row(p):
        return (p - len(WIDE)) % 2 == 1

    def payload(k, p):
        if p < len(WIDE):
            return y_wide.at[k, p, pl.ds(0, CAP)]
        rows = CAP + 1 if carries_odd_row(p) else CAP - 1
        return y_narrow.at[k, p - len(WIDE), pl.ds(0, rows)]

    def message(slot, p, chip, slot_there):
        return pltpu.make_async_remote_copy(
            payload(slot, p), payload(slot_there, p),
            send_sem, recv_sem.at[slot_there * N_PIECE + p],
            device_id=(chip,), device_id_type=pl.DeviceIdType.MESH)

    def wait_recv(slot, p):
        message(slot, p, me, slot).wait_recv()

    my_slot = jnp.where(me == C, 3, jnp.where(me == D, 2, 1))
    sent = []

    def multiply(p):
        e, c = PIECES[p]
        filled = jnp.broadcast_to(token[e], (ROWS, LANE)) < N_TOK
        if p < len(WIDE):
            w = w_first[:, pl.ds(c * LANE, 2 * LANE)] if e == 0 else w_wide[p - 2]
            y = jnp.dot(xs[e], w.astype(jnp.bfloat16), preferred_element_type=jnp.float32)
            low, high = (
                lax.bitcast_convert_type(
                    jnp.where(filled, v, 0.0).astype(jnp.bfloat16).astype(jnp.float32),
                    jnp.uint32)
                for v in (y[:, :LANE], y[:, LANE:]))
            y_wide[0, p] = (low >> 16) | high
            return None
        w = w_narrow[p - len(WIDE)]
        y = jnp.dot(xs[e], w.astype(jnp.bfloat16), preferred_element_type=jnp.float32)
        y = jnp.where(filled, y, 0.0)
        if carries_odd_row(p):
            tail = jnp.where(rank[ROWS - SUB:] == CAP, odd_row, y[ROWS - SUB:])
            y = jnp.concatenate([y[:ROWS - SUB], tail])
        y_narrow[0, p - len(WIDE)] = y.astype(jnp.bfloat16)
        return y[CAP - 1:CAP]

    def share(p):
        first = left if p in C_TO_A_VIA_D else jnp.where(me == C, A, left)
        for chip in (first, right):
            sent.append(message(0, p, chip, my_slot))
            sent[-1].start()

    locate(0, counts_of_expert(me * E_LOC))
    fetch_rows(0)
    fence()
    pl.when(me == B)(load_other_weights)
    near = counts_of_chips(me, jnp.where((me & 1) == 0, B, A))
    for e in range(1, E_LOC):
        locate(e, near[e])
    fetch_rows(1)
    fetch_rows(2)
    pl.when(me == A)(find_output_rows)

    w_copy(0).wait()
    wait_rows(0)
    multiply(0)
    pl.when(me != C)(lambda: pl.semaphore_wait(barrier, 2))
    pl.when(me == C)(lambda: pl.semaphore_wait(barrier, 3))
    share(0)
    fence()
    multiply(1)
    share(1)
    wait_rows(1)
    odd_row = None
    for p in range(2, N_PIECE):
        if p == 3:
            wait_rows(2)
            fetch_rows(3)
        if PIECES[p][0] not in xs:
            wait_rows(PIECES[p][0])
        w_copy(p).wait()
        odd_row = multiply(p)
        share(p)

    every = range(N_PIECE)
    a_passes = [(message(2, p, B, 2), message(1, p, D, 2)) for p in every]
    b_passes = {p: message(1, p, C, 3) for p in A_TO_C_VIA_B}
    c_sends = [message(0, p, B, 3) for p in every if p not in C_TO_A_VIA_D]
    d_to_a = {p: message(3, p, A, 3) for p in C_TO_A_VIA_D}
    d_to_c = {p: message(1, p, C, 3) for p in every if p not in A_TO_C_VIA_B}

    def pass_on(slot, copies):
        for p, copy in copies:
            wait_recv(slot, p)
            copy.start()

    @pl.when(me == D)
    def _():
        pass_on(3, list(d_to_a.items())[:2])
        pass_on(1, d_to_c.items())
        pass_on(3, list(d_to_a.items())[2:])

    pl.when(me == B)(lambda: pass_on(1, b_passes.items()))

    @pl.when(me == C)
    def _():
        for copy in c_sends:
            copy.start()

    pl.when(me != A)(find_output_rows)
    for copy in dst_copies:
        copy.wait()

    def store_rows(k, p):
        def put(piece, r, block, row):
            e, c = PIECES[piece]
            at = dst_s[k * LANE + e * ROWS + r] + SUB * (c + block)
            out_ref[pl.ds(at, 1), :] = row

        v = payload(k, p)[...]
        if p < len(WIDE):
            low = lax.bitcast_convert_type(v << 16, jnp.float32)
            high = lax.bitcast_convert_type(v & jnp.uint32(0xFFFF0000), jnp.float32)
            for r in range(CAP):
                put(p, r, 0, low[r:r + 1])
                put(p, r, 1, high[r:r + 1])
            return
        v = v.astype(jnp.float32)
        for r in range(CAP - 1):
            put(p, r, 0, v[r:r + 1])
        if carries_odd_row(p):
            put(p, CAP - 1, 0, v[CAP - 1:CAP])
            put(p - 1, CAP - 1, 0, v[CAP:CAP + 1])

    for p in every:
        wait_recv(2, p)
        pl.when(me == A)(a_passes[p][0].start)
        pl.when(me != (B if p in b_passes else D))(lambda: wait_recv(1, p))
        pl.when(me == A)(a_passes[p][1].start)
        for k in range(3):
            store_rows(k, p)

    def wait_sends(copies):
        for copy in copies:
            copy.wait_send()

    for p in LAST_SLOT_ORDER:
        if p == LAST_SLOT_ORDER[-4]:
            wait_sends(sent)
            pl.when(me == A)(lambda: wait_sends(sum(a_passes, ())))
            pl.when(me == B)(lambda: wait_sends(b_passes.values()))
            pl.when(me == C)(lambda: wait_sends(c_sends))
            pl.when(me == D)(lambda: wait_sends([*d_to_a.values(), *d_to_c.values()]))
        if p in d_to_a:
            pl.when(me != D)(lambda: wait_recv(3, p))
        else:
            wait_recv(3, p)
        store_rows(3, p)


def pallas_dist_moe_cap_ep_n512_d256_e4_h512_kernel(
    x: jax.Array,
    router_W: jax.Array,
    route_idx: jax.Array,
    expert_W: jax.Array,
):
    del router_W
    hbm = pl.BlockSpec(memory_space=pltpu.HBM)
    x_tiles = x.reshape(N_TOK // SUB, SUB, D_IN // LANE, LANE).transpose(0, 2, 1, 3)
    out = pl.pallas_call(
        _moe_kernel,
        out_shape=jax.ShapeDtypeStruct((N_TOK * D_OUT // LANE, LANE), jnp.float32),
        in_specs=[hbm, hbm, hbm],
        out_specs=pl.BlockSpec(memory_space=pltpu.VMEM),
        scratch_shapes=[
            pltpu.VMEM((N_BLK, LANE), jnp.int32),
            pltpu.VMEM((D_IN, D_OUT), jnp.float32),
            pltpu.VMEM((len(WIDE) - 2, D_IN, 2 * LANE), jnp.float32),
            pltpu.VMEM((len(NARROW), D_IN, LANE), jnp.float32),
            pltpu.VMEM((E_LOC, D_IN // LANE, ROWS, LANE), jnp.float32),
            pltpu.VMEM((SUB, LANE), jnp.int32),
            pltpu.SMEM((N_DEV * LANE,), jnp.int32),
            pltpu.VMEM((N_DEV, len(WIDE), ROWS, LANE), jnp.uint32),
            pltpu.VMEM((N_DEV, len(NARROW), ROWS, LANE), jnp.bfloat16),
            pltpu.SemaphoreType.DMA((N_PIECE,)),
            pltpu.SemaphoreType.DMA((E_LOC,)),
            pltpu.SemaphoreType.DMA,
            pltpu.SemaphoreType.DMA,
            pltpu.SemaphoreType.DMA((N_DEV * N_PIECE,)),
            pltpu.SemaphoreType.REGULAR,
        ],
        compiler_params=pltpu.CompilerParams(
            collective_id=0,
            disable_bounds_checks=True,
            disable_semaphore_checks=True,
            flags={"XLA_TPU_FORCE_LP_LLO_SCHEDULER": True},
        ),
    )(x_tiles, route_idx.reshape(N_BLK, LANE), expert_W)
    out = out.reshape(N_TOK // SUB, D_OUT // LANE, SUB, LANE).transpose(0, 2, 1, 3)
    return out.reshape(N_TOK, D_OUT)
```
